```python
import numpy as np

kernel_name = "dist_halo_stencil_i_m8192_n1024"

def setup_inputs():
    return {"x": np.random.randn(32768, 1024).astype(np.float32)}

def reference(x: np.ndarray) -> np.ndarray:
    out = np.empty_like(x)
    out[0] = x[0]
    out[-1] = x[-1]
    out[1:-1] = 0.25 * x[:-2] + 0.5 * x[1:-1] + 0.25 * x[2:]
    return out
```

```python
import jax
import jax.numpy as jnp
from jax import lax
from jax.experimental import pallas as pl
from jax.experimental.pallas import tpu as pltpu

N_DEV = 4
T = 8
G_ROWS = 128


def make(chunk_rows=256, blk=64, tail=(128, 64, 64), barrier_after=2, first_tile_at=None, mode="roll"):
  def kernel(x):
    m, n = x.shape
    half = m // 2
    groups = half // G_ROWS
    main_rows = m - sum(tail)
    n_main = main_rows // chunk_rows
    assert n_main * chunk_rows == main_rows
    n_chunks = n_main + len(tail)

    def body(x_hbm, o0, o1, buf, rsem, send_sems, recv_sems):
        me = lax.axis_index("i")
        left = (me + N_DEV - 1) % N_DEV
        right = (me + 1) % N_DEV
        barrier = pltpu.get_barrier_semaphore()
        for nb in (left, right):
            pl.semaphore_signal(barrier, 1, device_id=(nb,), device_id_type=pl.DeviceIdType.MESH)

        def read(lo, rows, c):
            return pltpu.make_async_copy(x_hbm.at[pl.ds(lo, rows)], buf.at[pl.ds(lo + T, rows)], rsem.at[c])

        def read_main(c):
            return read(pl.multiple_of(c * chunk_rows + T, T), chunk_rows, c)

        first = read(0, chunk_rows + T, 0)
        first.start()
        lax.fori_loop(1, n_main, lambda c, _: read_main(c).start(), None)
        tails = []
        s = main_rows
        for k, r in enumerate(tail):
            rows = r if k + 1 < len(tail) else r - T
            tails.append((read(s + T, rows, n_main + k), s, r))
            tails[-1][0].start()
            s += r

        def halo_copies():
            to_right = pltpu.make_async_remote_copy(
                x_hbm.at[pl.ds(m - T, T)], buf.at[pl.ds(0, T)], send_sems.at[0], recv_sems.at[0],
                device_id=(right,), device_id_type=pl.DeviceIdType.MESH)
            to_left = pltpu.make_async_remote_copy(
                x_hbm.at[pl.ds(0, T)], buf.at[pl.ds(m + T, T)], send_sems.at[1], recv_sems.at[1],
                device_id=(left,), device_id_type=pl.DeviceIdType.MESH)
            return to_right, to_left

        def stencil(r0, rows):
            if mode == "roll":
                v = buf[pl.ds(r0, rows + 2 * T), :]
                q = 0.25 * v
                up = pltpu.roll(q, 1, 0)[T:T + rows]
                dn = pltpu.roll(q, rows + 2 * T - 1, 0)[T:T + rows]
                return (up + 0.5 * v[T:T + rows]) + dn
            elif mode == "slice":
                w = buf.at[pl.ds(r0, rows + 2 * T)]
                return (0.25 * w[pl.ds(T - 1, rows), :] + 0.5 * w[pl.ds(T, rows), :]) + 0.25 * w[pl.ds(T + 1, rows), :]
            elif mode == "vslice":
                v = buf[pl.ds(r0, rows + 2 * T), :]
                q = 0.25 * v
                return (q[T - 1:T - 1 + rows] + 0.5 * v[T:T + rows]) + q[T + 1:T + 1 + rows]

        def compute_range(o, base, lo, cnt):
            def step(j, _):
                r0 = pl.multiple_of(lo + j * blk, T)
                rel = r0 - base
                o[rel // G_ROWS, pl.ds(pl.multiple_of(rel % G_ROWS, T), blk), :] = stencil(r0, blk)
            lax.fori_loop(0, cnt, step, None)

        first.wait()
        o0[0, pl.ds(T, blk - T), :] = stencil(T, blk - T)
        compute_range(o0, 0, blk, chunk_rows // blk - 1)

        n_half = half // chunk_rows

        def main_step(o, base):
            def f(c, _):
                read_main(c).wait()
                compute_range(o, base, c * chunk_rows, chunk_rows // blk)
            return f

        lax.fori_loop(1, barrier_after, main_step(o0, 0), None)
        pl.semaphore_wait(barrier, 2)
        to_right, to_left = halo_copies()
        to_right.start()
        to_left.start()
        lax.fori_loop(barrier_after, n_half, main_step(o0, 0), None)
        lax.fori_loop(n_half, n_main, main_step(o1, half), None)

        to_right.wait()
        to_left.wait()
        row = lax.broadcasted_iota(jnp.int32, (T, n), 0)
        v = stencil(0, T)
        o0[0, pl.ds(0, T), :] = jnp.where((row == 0) & (me == 0), buf[pl.ds(T, T), :], v)

        for k, (cp, s, r) in enumerate(tails):
            cp.wait()
            assert r % blk == 0 or blk % r == 0
            b = min(blk, r)
            last = k + 1 == len(tails)
            for j in range(r // b):
                r0 = s + j * b
                rel = r0 - half
                val = stencil(r0, b)
                if last and j + 1 == r // b:
                    rowb = lax.broadcasted_iota(jnp.int32, (b, n), 0)
                    val = jnp.where((rowb == b - 1) & (me == N_DEV - 1), buf[pl.ds(r0 + T, b), :], val)
                o1[rel // G_ROWS, pl.ds(rel % G_ROWS, b), :] = val

    o0, o1 = pl.pallas_call(
        body,
        out_shape=[pltpu.VMEM((groups, G_ROWS, n), x.dtype)] * 2,
        in_specs=[pl.BlockSpec(memory_space=pl.ANY)],
        out_specs=[pl.BlockSpec(memory_space=pltpu.VMEM)] * 2,
        scratch_shapes=[
            pltpu.VMEM((m + 2 * T, n), x.dtype),
            pltpu.SemaphoreType.DMA((n_chunks,)),
            pltpu.SemaphoreType.DMA((2,)),
            pltpu.SemaphoreType.DMA((2,)),
        ],
        compiler_params=pltpu.CompilerParams(collective_id=0, vmem_limit_bytes=40 * 1024 * 1024),
    )(x)
    return jnp.concatenate([o0, o1], axis=0).reshape(m, n)
  return kernel


pallas_dist_halo_stencil_i_m8192_n1024_kernel = make(mode="slice")
```

```python
import jax
import jax.numpy as jnp
from jax import lax
from jax.experimental import pallas as pl
from jax.experimental.pallas import tpu as pltpu

N_DEV = 4
T = 8
R = 256
J = R // T
P0, P2 = 4, 2
ZG = 2
MESH = pl.DeviceIdType.MESH


def make(X=384, SUB=16, D=6, f0=1, skips=(13, 22), cuts=(256, 480), cut_steps=(18, 28), RB=16,
         no_compute=False, dsc=True, K=3, units=((0, 8), (8, 8), (16, 8), (24, 4), (28, 2)), last_after=2,
         static_last=1, one_sided=True):
  def kernel(x):
    m, n = x.shape
    G = m // R
    GQ = G // P0
    GL = G - ZG
    w = n // P2
    S = X // SUB
    U0 = ZG * R - X
    NP = J - K
    edges = (U0,) + tuple(cuts) + (ZG * R,)
    n_b = len(edges) - 1
    assert all((e - U0) % SUB == 0 for e in edges) and R in edges
    done = (0,) + tuple((e - T) // RB for e in cuts)
    quarters = [(a * GQ, min(GQ, GL - a * GQ)) for a in range(P0)]
    last_bounce_step = f0 + S - 1
    for s_ in skips:
        if s_ <= last_bounce_step:
            last_bounce_step += 1
    assert last_bounce_step < NP, last_bounce_step

    def body(x_hbm, *refs):
        outs = [refs[a * P2:(a + 1) * P2] for a in range(P0)]
        buf, col_sems, unit_sems, rest_sem, raw_send, raw_recv, ret_send, ret_recv, halo_sems = refs[P0 * P2:]

        def tile_rows(c):
            return pl.ds(c * T if isinstance(c, int) else pl.multiple_of(c * T, T), T)

        def read_col(p):
            rows = tile_rows((p + J - 1) % J)
            return pltpu.make_async_copy(x_hbm.at[pl.ds(0, GL), rows], buf.at[pl.ds(ZG, GL), rows], col_sems.at[p])

        def read_unit(u, kk):
            g0, ng = units[u]
            rows = tile_rows(NP - 1 + kk)
            return pltpu.make_async_copy(x_hbm.at[pl.ds(g0, ng), rows], buf.at[pl.ds(ZG + g0, ng), rows],
                                         unit_sems.at[u * K + kk])

        rest = pltpu.make_async_copy(x_hbm.at[GL, pl.ds(0, U0)], buf.at[ZG + GL, pl.ds(0, U0)], rest_sem)
        rest.start()

        me = lax.axis_index("i")
        left = (me + N_DEV - 1) % N_DEV
        right = (me + 1) % N_DEV
        barrier = pltpu.get_barrier_semaphore()
        for nb in ((left,) if one_sided else (left, right)):
            pl.semaphore_signal(barrier, 1, device_id=(nb,), device_id_type=MESH)
        lax.fori_loop(0, D, lambda p, _: read_col(p).start(), None)
        pl.semaphore_wait(barrier, 1 if one_sided else 2)

        def sub(k):
            u = U0 + k * SUB
            return u, u // R, pl.ds(u % R if isinstance(u, int) else pl.multiple_of(u % R, T), SUB)

        def raw(k):
            _, z, rows = sub(k)
            return pltpu.make_async_remote_copy(x_hbm.at[GL + z, rows], buf.at[z, rows], raw_send, raw_recv.at[k],
                                                device_id=(right,), device_id_type=MESH)

        def ret(k):
            u, z, rows = sub(k)
            bi = sum(jnp.asarray(u >= e, jnp.int32) for e in cuts)
            return pltpu.make_async_remote_copy(buf.at[z, rows], buf.at[ZG + GL + z, rows], ret_send, ret_recv.at[bi],
                                                device_id=(left,), device_id_type=MESH)

        def bounce(k):
            raw(k).wait_recv()
            ret(k).start()

        def wait_batch(i):
            lo, hi = edges[i], edges[i + 1]
            v = buf.at[ZG + GL + lo // R, pl.ds(lo % R, hi - lo)]
            pltpu.make_async_copy(v, v, ret_recv.at[i]).wait()

        lax.fori_loop(0, S, lambda k, _: raw(k).start(), None)
        halo = pltpu.make_async_remote_copy(x_hbm.at[0, pl.ds(0, T)], buf.at[ZG + G, pl.ds(0, T)],
                                            halo_sems.at[0], halo_sems.at[1], device_id=(left,), device_id_type=MESH)

        def column(g0, ng, c):
            if no_compute:
                return
            a = g0 // GQ
            first, last = c == 0, c == J - 1
            if not isinstance(c, int):
                first, last = first.astype(jnp.int32), last.astype(jnp.int32)
            rows = tile_rows(c)
            sub_i = lax.broadcasted_iota(jnp.int32, (ng, T, w), 1)
            for b in range(P2):
                cs = pl.ds(b * w, w)
                cur = buf[pl.ds(ZG + g0, ng), rows, cs]
                prev = buf[pl.ds(ZG + g0 - first, ng), tile_rows((c + J - 1) % J), cs]
                nxt = buf[pl.ds(ZG + g0 + last, ng), tile_rows((c + 1) % J), cs]
                up = pltpu.roll(jnp.where(sub_i == T - 1, prev, cur), 1, 1)
                dn = pltpu.roll(jnp.where(sub_i == 0, nxt, cur), T - 1, 1)
                outs[a][b][pl.ds(g0 - a * GQ, ng), rows, :] = (0.25 * up + 0.5 * cur) + 0.25 * dn

        def block(f, rows, keep=None):
            if no_compute:
                return
            static = isinstance(f, int)

            def loc(r):
                r = r + ZG * R
                return r // R, (r % R if static else pl.multiple_of(r % R, T))

            (g, o), (gp, op), (gn, on) = loc(f), loc(f - T), loc(f + rows)
            a = 0 if static and f == 0 else P0 - 1
            for b in range(P2):
                cs = pl.ds(b * w, w)
                cur = buf[g, pl.ds(o, rows), cs]
                q = 0.25 * jnp.concatenate([buf[gp, pl.ds(op, T), cs], cur, buf[gn, pl.ds(on, T), cs]], axis=0)
                up = pltpu.roll(q, 1, 0)[T:T + rows]
                dn = pltpu.roll(q, rows + 2 * T - 1, 0)[T:T + rows]
                val = (up + 0.5 * cur) + dn
                if keep is not None:
                    val = jnp.where(keep, cur, val)
                outs[a][b][g - ZG - a * GQ, pl.ds(o, rows), :] = val

        def rest_blocks(lo, hi):
            lax.fori_loop(lo, hi, lambda i, _: block(GL * R + i * RB, RB), None)

        for p in range(2):
            if p >= f0:
                bounce(p - f0)
                if p == f0:
                    halo.start()
            read_col(p).wait()
            read_col(D + p).start()
        rest.wait()

        def step(p, _):
            k = p - f0 - sum(jnp.asarray(p > s_, jnp.int32) for s_ in skips)
            go = (k >= 0) & (k < S)
            for s_ in skips:
                go = go & (p != s_)

            @pl.when(go)
            def _():
                bounce(k)

            if f0 >= 2:
                pl.when(p == f0)(lambda: halo.start())

            read_col(p).wait()

            @pl.when(p + D < NP)
            def _():
                read_col(p + D).start()

            for u in range(len(units)):
                @pl.when(p == min(NP - D + u, NP - 1))
                def _(u=u):
                    for kk in range(K):
                        read_unit(u, kk).start()

            c = p - 2
            pl.when(c != 0)(lambda: column(0, 1, c))
            column(1, GQ - 1, c)
            for g0, ng in quarters[1:]:
                column(g0, ng, c)

            lo = hi = 0
            for i, ps in enumerate(cut_steps):
                pl.when(p == ps)(lambda i=i: wait_batch(i))
                lo = jnp.where(p == ps, done[i], lo)
                hi = jnp.where(p == ps, done[i + 1], hi)
            rest_blocks(lo, hi)

        lax.fori_loop(2, NP, step, None)

        row = lax.broadcasted_iota(jnp.int32, (T, w), 0)
        block(0, T, keep=(row == 0) & (me == 0))
        lax.fori_loop(0, S, lambda k, _: raw(k).wait_send(), None)

        def finish_rest():
            wait_batch(n_b - 1)
            halo.wait()
            rest_blocks(done[-1], ZG * R // RB - 1)
            rowb = lax.broadcasted_iota(jnp.int32, (RB, w), 0)
            block(m - RB, RB, keep=(rowb == RB - 1) & (me == N_DEV - 1))
            lax.fori_loop(0, S, lambda k, _: ret(k).wait_send(), None)

        for u, (g0, ng) in enumerate(units):
            if u == last_after:
                finish_rest()
            if u >= len(units) - static_last:
                for c in range(NP - 2, J):
                    if c - (NP - 2) < K:
                        read_unit(u, c - (NP - 2)).wait()
                    column(g0, ng, c)
                continue

            def unit_step(c, _, u=u, g0=g0, ng=ng):
                for kk in range(K):
                    pl.when(c == NP - 2 + kk)(lambda kk=kk: read_unit(u, kk).wait())
                column(g0, ng, c)
            lax.fori_loop(NP - 2, J, unit_step, None)

    outs = pl.pallas_call(
        body,
        out_shape=[pltpu.VMEM((GQ, R, w), x.dtype)] * (P0 * P2),
        in_specs=[pl.BlockSpec(memory_space=pl.ANY)],
        out_specs=[pl.BlockSpec(memory_space=pltpu.VMEM)] * (P0 * P2),
        scratch_shapes=[
            pltpu.VMEM((ZG + G + 1, R, n), x.dtype),
            pltpu.SemaphoreType.DMA((NP,)),
            pltpu.SemaphoreType.DMA((len(units) * K,)),
            pltpu.SemaphoreType.DMA(()),
            pltpu.SemaphoreType.DMA(()),
            pltpu.SemaphoreType.DMA((S,)),
            pltpu.SemaphoreType.DMA(()),
            pltpu.SemaphoreType.DMA((n_b,)),
            pltpu.SemaphoreType.DMA((2,)),
        ],
        compiler_params=pltpu.CompilerParams(collective_id=0, vmem_limit_bytes=40 * 1024 * 1024,
                                             disable_semaphore_checks=dsc),
    )(x.reshape(G, R, n))
    rows = [jnp.concatenate(outs[a * P2:(a + 1) * P2], axis=2) for a in range(P0)]
    return jnp.concatenate(rows, axis=0).reshape(m, n)
  return kernel


pallas_dist_halo_stencil_i_m8192_n1024_kernel = make(X=400)
```

```python
import jax
import jax.numpy as jnp
from jax import lax
from jax.experimental import pallas as pl
from jax.experimental.pallas import tpu as pltpu

N_DEV = 4
MESH = pl.DeviceIdType.MESH

T = 8
R = 256
J = R // T
P0, P2 = 4, 2
ZG = 2

X = 400
SUB = 16
S = X // SUB
U0 = ZG * R - X
RB = 16

DEPTH = 6
K = 3
NP = J - K
UNITS = ((0, 8), (8, 8), (16, 8), (24, 4), (28, 2))
UNROLLED_UNITS = 3

EDGES = (U0, 256, 448, 496, ZG * R)
BATCH_STEPS = (18, 28)
BATCH_UNITS = (2, 3)
BLOCKS_DONE = (0,) + tuple((e - T) // RB for e in EDGES[1:-1])


def pallas_dist_halo_stencil_i_m8192_n1024_kernel(x: jax.Array):
    m, n = x.shape
    groups = m // R
    gq = groups // P0
    gl = groups - ZG
    w = n // P2
    n_batches = len(EDGES) - 1
    assert m == groups * R and sum(ng for _, ng in UNITS) == gl and S < NP

    def body(x_hbm, *refs):
        outs = [refs[a * P2:(a + 1) * P2] for a in range(P0)]
        (buf, col_sems, unit_sems, rest_sem, raw_send, raw_recv, ret_send,
         ret_recv, halo_sems, hello_sem) = refs[P0 * P2:]

        def aligned(r):
            return r if isinstance(r, int) else pl.multiple_of(r, T)

        def tile_rows(c):
            return pl.ds(aligned(c * T), T)

        def read_col(p):
            rows = tile_rows((p + J - 1) % J)
            return pltpu.make_async_copy(
                x_hbm.at[pl.ds(0, gl), rows], buf.at[pl.ds(ZG, gl), rows],
                col_sems.at[p])

        def read_unit(u, i):
            g0, ng = UNITS[u]
            rows = tile_rows(NP - 1 + i)
            return pltpu.make_async_copy(
                x_hbm.at[pl.ds(g0, ng), rows], buf.at[pl.ds(ZG + g0, ng), rows],
                unit_sems.at[u * K + i])

        rest = pltpu.make_async_copy(
            x_hbm.at[gl, pl.ds(0, U0)], buf.at[ZG + gl, pl.ds(0, U0)], rest_sem)
        rest.start()

        me = lax.axis_index("i")
        left = (me + N_DEV - 1) % N_DEV
        right = (me + 1) % N_DEV
        barrier = pltpu.get_barrier_semaphore()
        pl.semaphore_signal(barrier, 1, device_id=(left,), device_id_type=MESH)
        lax.fori_loop(0, DEPTH, lambda p, _: read_col(p).start(), None)
        pl.semaphore_wait(barrier, 1)

        def sub_rows(k):
            u = U0 + k * SUB
            return u, u // R, pl.ds(aligned(u % R), SUB)

        def raw(k):
            _, z, rows = sub_rows(k)
            return pltpu.make_async_remote_copy(
                x_hbm.at[gl + z, rows], buf.at[z, rows],
                raw_send.at[z], raw_recv.at[k],
                device_id=(right,), device_id_type=MESH)

        def bounce(k):
            raw(k).wait_recv()
            u, z, rows = sub_rows(k)
            batch = sum(jnp.asarray(u >= e, jnp.int32) for e in EDGES[1:-1])
            pltpu.make_async_remote_copy(
                buf.at[z, rows], buf.at[ZG + gl + z, rows],
                ret_send.at[z], ret_recv.at[batch],
                device_id=(left,), device_id_type=MESH).start()

        def wait_batch(i):
            lo, hi = EDGES[i], EDGES[i + 1]
            rows = buf.at[ZG + gl + lo // R, pl.ds(lo % R, hi - lo)]
            pltpu.make_async_copy(rows, rows, ret_recv.at[i]).wait()

        def wait_sent(src, g0, send_sems):
            for z, rows in enumerate((pl.ds(U0, R - U0), pl.ds(0, R))):
                pltpu.make_async_remote_copy(
                    src.at[g0 + z, rows], buf.at[ZG + gl + z, rows],
                    send_sems.at[z], halo_sems.at[1],
                    device_id=(left,), device_id_type=MESH).wait_send()

        lax.fori_loop(0, S, lambda k, _: raw(k).start(), None)
        pl.semaphore_signal(hello_sem, 1, device_id=(right,), device_id_type=MESH)
        halo = pltpu.make_async_remote_copy(
            x_hbm.at[0, pl.ds(0, T)], buf.at[ZG + groups, pl.ds(0, T)],
            halo_sems.at[0], halo_sems.at[1],
            device_id=(left,), device_id_type=MESH)

        def column(g0, ng, c):
            a = g0 // gq
            first, last = c == 0, c == J - 1
            if not isinstance(c, int):
                first, last = first.astype(jnp.int32), last.astype(jnp.int32)
            rows = tile_rows(c)
            above, below = tile_rows((c + J - 1) % J), tile_rows((c + 1) % J)
            sublane = lax.broadcasted_iota(jnp.int32, (ng, T, w), 1)
            for b in range(P2):
                cols = pl.ds(b * w, w)
                cur = buf[pl.ds(ZG + g0, ng), rows, cols]
                prev = buf[pl.ds(ZG + g0 - first, ng), above, cols]
                nxt = buf[pl.ds(ZG + g0 + last, ng), below, cols]
                up = pltpu.roll(jnp.where(sublane == T - 1, prev, cur), 1, 1)
                dn = pltpu.roll(jnp.where(sublane == 0, nxt, cur), T - 1, 1)
                outs[a][b][pl.ds(g0 - a * gq, ng), rows, :] = (
                    (0.25 * up + 0.5 * cur) + 0.25 * dn)

        def block(a, r0, rows, keep=None):
            def locate(r):
                return (r + ZG * R) // R, aligned(r % R)

            (g, o), (gp, op), (gn, on) = locate(r0), locate(r0 - T), locate(r0 + rows)
            for b in range(P2):
                cols = pl.ds(b * w, w)
                cur = buf[g, pl.ds(o, rows), cols]
                q = 0.25 * jnp.concatenate(
                    [buf[gp, pl.ds(op, T), cols], cur, buf[gn, pl.ds(on, T), cols]],
                    axis=0)
                up = pltpu.roll(q, 1, 0)[T:T + rows]
                dn = pltpu.roll(q, rows + 2 * T - 1, 0)[T:T + rows]
                val = (up + 0.5 * cur) + dn
                if keep is not None:
                    val = jnp.where(keep, cur, val)
                outs[a][b][g - ZG - a * gq, pl.ds(o, rows), :] = val

        def rest_blocks(lo, hi):
            lax.fori_loop(
                lo, hi, lambda i, _: block(P0 - 1, gl * R + i * RB, RB), None)

        read_col(0).wait()
        read_col(DEPTH).start()
        pl.semaphore_wait(hello_sem, 1)
        bounce(0)
        halo.start()
        read_col(1).wait()
        read_col(DEPTH + 1).start()
        rest.wait()

        def step(p, _):
            pl.when(p <= S)(lambda: bounce(p - 1))
            read_col(p).wait()
            pl.when(p + DEPTH < NP)(lambda: read_col(p + DEPTH).start())
            for u in range(len(UNITS)):
                @pl.when(p == min(NP - DEPTH + u, NP - 1))
                def _(u=u):
                    for i in range(K):
                        read_unit(u, i).start()

            c = p - 2
            pl.when(c != 0)(lambda: column(0, 1, c))
            column(1, gq - 1, c)
            for g0 in range(gq, gl, gq):
                column(g0, min(gq, gl - g0), c)

            lo = hi = 0
            for i, at in enumerate(BATCH_STEPS):
                pl.when(p == at)(lambda i=i: wait_batch(i))
                lo = jnp.where(p == at, BLOCKS_DONE[i], lo)
                hi = jnp.where(p == at, BLOCKS_DONE[i + 1], hi)
            rest_blocks(lo, hi)

        lax.fori_loop(2, NP, step, None)

        row = lax.broadcasted_iota(jnp.int32, (T, w), 0)
        block(0, 0, T, keep=(row == 0) & (me == 0))
        wait_sent(x_hbm, gl, raw_send)
        halo.wait()

        for u, (g0, ng) in enumerate(UNITS):
            if u in BATCH_UNITS:
                i = len(BATCH_STEPS) + BATCH_UNITS.index(u)
                wait_batch(i)
                if i + 1 < n_batches:
                    rest_blocks(BLOCKS_DONE[i], BLOCKS_DONE[i + 1])
                else:
                    for r0 in range(gl * R + BLOCKS_DONE[i] * RB, m - RB, RB):
                        block(P0 - 1, r0, RB)
                    row = lax.broadcasted_iota(jnp.int32, (RB, w), 0)
                    block(P0 - 1, m - RB, RB,
                          keep=(row == RB - 1) & (me == N_DEV - 1))
                    wait_sent(buf, 0, ret_send)

            if u >= len(UNITS) - UNROLLED_UNITS:
                for c in range(NP - 2, J):
                    if c < NP - 2 + K:
                        read_unit(u, c - (NP - 2)).wait()
                    column(g0, ng, c)
            else:
                def unit_step(c, _, u=u, g0=g0, ng=ng):
                    for i in range(K):
                        pl.when(c == NP - 2 + i)(lambda i=i: read_unit(u, i).wait())
                    column(g0, ng, c)

                lax.fori_loop(NP - 2, J, unit_step, None)

    dma = pltpu.SemaphoreType.DMA
    pieces = pl.pallas_call(
        body,
        out_shape=[pltpu.VMEM((gq, R, w), x.dtype)] * (P0 * P2),
        in_specs=[pl.BlockSpec(memory_space=pltpu.HBM)],
        out_specs=[pl.BlockSpec(memory_space=pltpu.VMEM)] * (P0 * P2),
        scratch_shapes=[
            pltpu.VMEM((ZG + groups + 1, R, n), x.dtype),
            dma((NP,)),
            dma((len(UNITS) * K,)),
            dma(()),
            dma((ZG,)), dma((S,)),
            dma((ZG,)), dma((n_batches,)),
            dma((2,)),
            pltpu.SemaphoreType.REGULAR,
        ],
        compiler_params=pltpu.CompilerParams(
            collective_id=0,
            vmem_limit_bytes=40 * 1024 * 1024,
            disable_semaphore_checks=True,
        ),
    )(x.reshape(groups, R, n))
    bands = [jnp.concatenate(pieces[a * P2:(a + 1) * P2], axis=2) for a in range(P0)]
    return jnp.concatenate(bands, axis=0).reshape(m, n)
```
